```python
import numpy as np

kernel_name = "dist_ar_i_i_m2048_n512"

def setup_inputs():
    return {"x": np.random.randn(8192, 512).astype(np.float32)}

def reference(x: np.ndarray) -> np.ndarray:
    return x.reshape(4, 2048, 512).sum(axis=0)
```

```python
import functools

import jax
import jax.numpy as jnp
from jax import lax
from jax.experimental import pallas as pl
from jax.experimental.pallas import tpu as pltpu

_MESH = pl.DeviceIdType.MESH
_BF = jnp.bfloat16
_F32 = jnp.float32

_SHIFT = 16
_B1 = (16, 48, 128, 256, 384)
_B2 = (128, 256, 384)
_B3 = (128, 256, 384)
_EARLY = 3
_RB = 32


def _split(total, bounds):
    bs = [0] + [b for b in bounds if b < total] + [total]
    return [(bs[i], bs[i + 1] - bs[i]) for i in range(len(bs) - 1)]


def _rowloop(o, s, f):
    nb, rem = divmod(s, _RB)
    if nb <= 2:
        for i in range(nb):
            f(o + i * _RB, _RB)
    else:
        def step(i, c):
            f(pl.multiple_of(o + i * _RB, 16), _RB)
            return c
        lax.fori_loop(0, nb, step, 0)
    if rem:
        f(o + nb * _RB, rem)


def pallas_dist_ar_i_i_m2048_n512_kernel(x: jax.Array):
    m, n = x.shape
    q = m // 4
    r = _SHIFT
    qs = (q - r, q + r)
    qo = ((0, q - r), (2 * q, 3 * q - r))
    ch1 = [_split(qs[k], _B1) for k in range(2)]
    ch2 = [_split(qs[k], _B2) for k in range(2)]
    ch3 = [_split(qs[k], _B3) for k in range(2)]
    n1 = max(len(c) for c in ch1)
    n2 = max(len(c) for c in ch2)
    n3 = max(len(c) for c in ch3)

    def body(x_ref, o_ref, xs, xk, s1, r1, s2, r2,
             lsem_s, lsem_k, ss1, rs1, ss2, rs2, ss3, rs3, hsem):
        pid = lax.axis_index("i")
        bar = pltpu.get_barrier_semaphore()

        def rc(src, dst, ss, rs, dev):
            return pltpu.make_async_remote_copy(
                src_ref=src, dst_ref=dst, send_sem=ss, recv_sem=rs,
                device_id=(dev,), device_id_type=_MESH)

        def program(p):
            py, px = p ^ 1, 3 - p
            kk = ((p ^ (p >> 1)) & 1, p >> 1)
            outer, inner = (py, px), (px, py)
            order = (1, 0) if p == 3 else (0, 1)
            keep = [qo[h][kk[h]] for h in range(2)]
            send = [qo[h][1 - kk[h]] for h in range(2)]
            cs1 = [ch1[1 - kk[h]] for h in range(2)]
            cr1 = [ch1[kk[h]] for h in range(2)]
            c2 = [ch2[kk[h]] for h in range(2)]
            cs3 = [ch3[kk[h]] for h in range(2)]
            cr3 = [ch3[1 - kk[h]] for h in range(2)]

            if p != 2:
                for h in order:
                    pl.semaphore_signal(bar, inc=1, device_id=(outer[h],),
                                        device_id_type=_MESH)

            ld_s = [[pltpu.make_async_copy(
                x_ref.at[pl.ds(send[h] + o, s)], xs.at[h, pl.ds(o, s)],
                lsem_s.at[h * n1 + c]) for c, (o, s) in enumerate(cs1[h])]
                for h in range(2)]
            ld_k = [[pltpu.make_async_copy(
                x_ref.at[pl.ds(keep[h] + o, s)], xk.at[h, pl.ds(o, s)],
                lsem_k.at[h * n2 + c]) for c, (o, s) in enumerate(c2[h])]
                for h in range(2)]

            def ph1(chunks):
                return [[rc(s1.at[h, pl.ds(o, s)], r1.at[h, pl.ds(o, s)],
                            ss1.at[h * n1 + c], rs1.at[h * n1 + c], outer[h])
                         for c, (o, s) in enumerate(chunks[h])] for h in range(2)]

            def ph3(base, chunks):
                return [[rc(o_ref.at[pl.ds(base[h] + o, s)],
                            o_ref.at[pl.ds(base[h] + o, s)],
                            ss3.at[h * n3 + c], rs3.at[h * n3 + c], outer[h])
                         for c, (o, s) in enumerate(chunks[h])] for h in range(2)]

            d1, d1r = ph1(cs1), ph1(cr1)
            d2 = [[rc(s2.at[h, pl.ds(o, s)], r2.at[h, pl.ds(o, s)],
                      ss2.at[h * n2 + c], rs2.at[h * n2 + c], inner[h])
                   for c, (o, s) in enumerate(c2[h])] for h in range(2)]
            d3, d3r = ph3(keep, cs3), ph3(send, cr3)

            if p in (1, 3):
                seq = [(h, c) for h in order for c in range(_EARLY)]
                held = range(_EARLY, 2 * _EARLY)
            else:
                seq = [(h, c) for c in range(_EARLY) for h in order]
                held = range(2 * _EARLY) if p == 0 else range(0)
            seq += [(h, c) for c in range(_EARLY, n1) for h in order
                    if c < len(cs1[h])]
            for h, c in seq:
                ld_s[h][c].start()

            if p == 2:
                pl.semaphore_wait(bar, 2)
                for h in order:
                    pl.semaphore_signal(hsem, inc=1, device_id=(outer[h],),
                                        device_id_type=_MESH)
            elif p != 0:
                pl.semaphore_wait(bar, 1)

            for i, (h, c) in enumerate(seq):
                o, s = cs1[h][c]
                ld_s[h][c].wait()

                def cast(row, cnt, h=h):
                    s1[h, pl.ds(row, cnt), :] = (
                        xs[h, pl.ds(row, cnt), :].astype(_BF))
                _rowloop(o, s, cast)
                if i not in held:
                    d1[h][c].start()
                elif i == held[-1]:
                    if p == 0:
                        pl.semaphore_wait(bar, 2)
                    else:
                        pl.semaphore_wait(hsem, 1)
                    for j in held:
                        d1[seq[j][0]][seq[j][1]].start()

            for c in range(n2):
                for h in order:
                    if c < len(c2[h]):
                        ld_k[h][c].start()

            got = [0, 0]
            for c in range(n2):
                for h in order:
                    if c >= len(c2[h]):
                        continue
                    o, s = c2[h][c]
                    ld_k[h][c].wait()
                    while got[h] < len(cr1[h]) and cr1[h][got[h]][0] < o + s:
                        d1r[h][got[h]].wait_recv()
                        got[h] += 1

                    def add1(row, cnt, h=h):
                        s2[h, pl.ds(row, cnt), :] = (
                            xk[h, pl.ds(row, cnt), :]
                            + r1[h, pl.ds(row, cnt), :].astype(_F32)).astype(_BF)
                    _rowloop(o, s, add1)
                    d2[h][c].start()
            for h in order:
                for d in d1[h]:
                    d.wait_send()

            got = [0, 0]
            for c in range(n3):
                for h in order[::-1]:
                    if c >= len(cs3[h]):
                        continue
                    o, s = cs3[h][c]
                    while got[h] < len(c2[h]) and c2[h][got[h]][0] < o + s:
                        d2[h][got[h]].wait_recv()
                        got[h] += 1

                    def add2(row, cnt, h=h):
                        o_ref[pl.ds(pl.multiple_of(keep[h] + row, 16), cnt), :] = (
                            s2[h, pl.ds(row, cnt), :].astype(_F32)
                            + r2[h, pl.ds(row, cnt), :].astype(_F32)).astype(_BF)
                    _rowloop(o, s, add2)
                    d3[h][c].start()
            for h in order:
                for d in d2[h]:
                    d.wait_send()
            for h in order:
                for d in d3[h]:
                    d.wait_send()
            for h in order:
                for d in d3r[h]:
                    d.wait_recv()

        for p in range(4):
            pl.when(pid == p)(functools.partial(program, p))

    qm = q + r
    dma = pltpu.SemaphoreType.DMA
    return pl.pallas_call(
        body,
        out_shape=jax.ShapeDtypeStruct((m, n), _BF),
        in_specs=[pl.BlockSpec(memory_space=pl.ANY)],
        out_specs=pl.BlockSpec(memory_space=pltpu.VMEM),
        scratch_shapes=[
            pltpu.VMEM((2, qm, n), _F32), pltpu.VMEM((2, qm, n), _F32),
            pltpu.VMEM((2, qm, n), _BF), pltpu.VMEM((2, qm, n), _BF),
            pltpu.VMEM((2, qm, n), _BF), pltpu.VMEM((2, qm, n), _BF),
            dma((2 * n1,)), dma((2 * n2,)),
            dma((2 * n1,)), dma((2 * n1,)),
            dma((2 * n2,)), dma((2 * n2,)),
            dma((2 * n3,)), dma((2 * n3,)),
            pltpu.SemaphoreType.REGULAR,
        ],
        compiler_params=pltpu.CompilerParams(
            collective_id=0,
            vmem_limit_bytes=32 * 1024 * 1024,
            disable_semaphore_checks=True,
        ),
    )(x)
```

```python
import functools

import jax
import jax.numpy as jnp
from jax import lax
from jax.experimental import pallas as pl
from jax.experimental.pallas import tpu as pltpu

_MESH = pl.DeviceIdType.MESH
_BF = jnp.bfloat16
_F32 = jnp.float32
_I32 = jnp.int32

_EXP = 0x7F807F80
_TOP = 0x80008000
_NIB = 0x07800780
_B11 = 0x08000800
_KEEP = 0x87FF87FF


def _c(v):
    return jnp.int32(v - (1 << 32) if v >= (1 << 31) else v)


def _sh(x, k):
    amount = jnp.full(x.shape, abs(k), x.dtype)
    return lax.shift_left(x, amount) if k >= 0 else lax.shift_right_logical(x, amount)


def _cb(x, i):
    return x[:, 128 * i:128 * i + 128]


def _tile4(x):
    return jnp.concatenate([x] * 4, axis=1)


def _pack16(vb):
    u = lax.bitcast_convert_type(vb.astype(_F32), _I32)
    return u[:8] | _sh(u[8:], -16)


def _unpack16(w):
    hi = lax.bitcast_convert_type(w & _c(0xFFFF0000), _F32)
    lo = lax.bitcast_convert_type(_sh(w, 16), _F32)
    return jnp.concatenate([hi, lo], axis=0)


def _encode(ws, put, flag):
    mx = None
    for w in ws:
        x = w & _c(_EXP)
        x = jnp.maximum(x, _sh(x, 16))
        mx = x if mx is None else jnp.maximum(mx, x)
    mx = jnp.maximum(jnp.maximum(_cb(mx, 0), _cb(mx, 1)),
                     jnp.maximum(_cb(mx, 2), _cb(mx, 3)))
    base = jnp.maximum(_sh(mx, -23) - 31, 0)
    bb = _sh(base, 7) | _sh(base, 23)
    bb4 = _tile4(bb)
    cc4 = _tile4(_c(_EXP) - bb)
    bad = None
    acc = [None] * ((len(ws) + 3) // 4)
    for rb, w in enumerate(ws):
        x = w & _c(_EXP)
        m = (x + cc4) & _c(_TOP)
        m = m - _sh(m, -15)
        wp = w - (bb4 & m)
        b = x & ~m
        bad = b if bad is None else bad | b
        q = 4 * (rb % 4)
        r = _sh(wp + _c(_NIB), q - 11) & _c(0x00010001 << q)
        acc[rb // 4] = r if acc[rb // 4] is None else acc[rb // 4] | r
        d = _cb(wp, 3)
        put(3 * rb, (_cb(wp, 0) & _c(_KEEP)) | (_sh(d, 11) & 0x78007800))
        put(3 * rb + 1, (_cb(wp, 1) & _c(_KEEP)) | (_sh(d, 7) & 0x78007800))
        put(3 * rb + 2, (_cb(wp, 2) & _c(_KEEP)) | (_sh(d, 3) & 0x38003800)
            | (_sh(d, -1) & 0x40004000))
    flag = flag | _cb(bad, 0) | _cb(bad, 1) | _cb(bad, 2) | _cb(bad, 3)
    meta = None
    for i, a in enumerate(acc):
        plane = _cb(a, 0) | _sh(_cb(a, 1), 1) | _sh(_cb(a, 2), 2) | _sh(_cb(a, 3), 3)
        for t in range(2):
            low = plane & (0 - plane)
            plane = plane ^ low
            e = _sh(lax.bitcast_convert_type(low.astype(_F32), _I32), -23) & 0xFF
            pos = _sh(jnp.maximum(e - 126, 0), 8 + 12 * i + 6 * t)
            meta = pos if meta is None else meta | pos
        flag = flag | plane
    put(3 * len(ws), meta | jnp.where(flag != 0, 255, base))
    return flag


def _decode(get, put_w, nrb, flag):
    meta = get(3 * nrb)
    base = meta & 0xFF
    flag = flag | _sh(base + 1, -8)
    bb4 = _tile4(_sh(base, 7) | _sh(base, 23))
    planes = []
    for i in range((nrb + 3) // 4):
        plane = None
        for t in range(2):
            pos = _sh(meta, -(8 + 12 * i + 6 * t)) & 63
            bit = jnp.where(
                pos > 0, lax.shift_left(jnp.ones_like(pos), (pos - 1) & 31), 0)
            plane = bit if plane is None else plane | bit
        planes.append(jnp.concatenate([_sh(plane, -n) for n in range(4)], axis=1))
    for rb in range(nrb):
        o0, o1, o2 = get(3 * rb), get(3 * rb + 1), get(3 * rb + 2)
        d = ((_sh(o0, -11) & 0x000F000F) | (_sh(o1, -7) & 0x00F000F0)
             | (_sh(o2, -3) & 0x07000700) | (_sh(o2, 1) & _c(_TOP)))
        wn = jnp.concatenate(
            [o0 & _c(_KEEP), o1 & _c(_KEEP), o2 & _c(_KEEP), d], axis=1)
        r = _sh(planes[rb // 4], 11 - 4 * (rb % 4))
        z = (wn & _c(_NIB)) + _c(_NIB)
        m = (z | r) & _c(_B11)
        m = _sh(m, 4) - _sh(m, -11)
        put_w(rb, wn + ((z ^ r) & _c(_B11)) + (bb4 & m))
    return flag


_M, _N = 2048, 512
_HM = _M // 2
_RAW = 16
_NRB = (3, 8)
_NU = 3
_CS = 384


def pallas_dist_ar_i_i_m2048_n512_kernel(x: jax.Array):
    assert x.shape == (_M, _N)

    def body(x_ref, o_ref, xv, pus, pur, pls, plr, own2, t1s, t1r, t2s, t2r,
             fl_ref, f1s, f1r, f2s, f2r,
             lsem, ksem, ss, rs, tss, trs, fss, frs, hsem):
        p = lax.axis_index("i")
        py, px = p ^ 1, 3 - p
        yc, xc = (p ^ (p >> 1)) & 1, p >> 1
        flip = (p + 1) >> 2
        odd = (p & 1) == 1
        bar = pltpu.get_barrier_semaphore()
        psend, precv = (pus, pls), (pur, plr)
        cols = (pl.ds(0, _CS), pl.ds(_CS, _N - _CS))

        def half(j):
            h = j ^ flip
            kk = jnp.where(h == 0, yc, xc)
            outer = jnp.where(h == 0, py, px)
            inner = jnp.where(h == 0, px, py)
            return h, kk, outer, inner

        hv = [half(j) for j in range(2)]

        def row(z, h, k, i):
            r = (16 + 480 * k + 48 * i) if z == 0 else (112 + 528 * k + 128 * i)
            return pl.multiple_of(h * _HM + r, 16)

        def raw_rows(h):
            return pl.ds(pl.multiple_of(h * _HM, 16), _RAW)

        def blk(r0, rb):
            return pl.ds(pl.multiple_of(r0 + 16 * rb, 16), 16)

        def wblk(r0, rb):
            return pl.ds(pl.multiple_of((r0 >> 1) + 8 * rb, 8), 8)

        def rc(src, dst, s_sem, r_sem, dev):
            return pltpu.make_async_remote_copy(
                src_ref=src, dst_ref=dst, send_sem=s_sem, recv_sem=r_sem,
                device_id=(dev,), device_id_type=_MESH)

        def slot(ph, h, i):
            return (ph * 2 + h) * _NU + i

        def unit_copy(ph, z, h, i, dev):
            s = slot(ph, h, i)
            return rc(psend[z].at[s], precv[z].at[s],
                      ss.at[z * 6 * _NU + s], rs.at[z * 6 * _NU + s], dev)

        def raw_copy(ph, h, k, dev):
            if ph == 2:
                src = dst = o_ref.at[raw_rows(h), cols[k]]
            else:
                src, dst = ((t1s, t1r), (t2s, t2r))[ph]
                src, dst = src.at[h, :, cols[k]], dst.at[h, :, cols[k]]
            return rc(src, dst, tss.at[ph * 2 + h], trs.at[ph * 2 + h], dev)

        def load(r0, n, sem):
            return pltpu.make_async_copy(
                x_ref.at[pl.ds(r0, n)], xv.at[pl.ds(r0, n)], sem)

        def unit_load(z, h, k, i):
            return load(row(z, h, k, i), 16 * _NRB[z],
                        lsem.at[2 + (z * 2 + h) * _NU + i])

        def raw_load(h):
            return load(pl.multiple_of(h * _HM, 16), _RAW, lsem.at[h])

        def pieces(sent, f):
            for h, kk, outer, inner in hv:
                for k in range(2):
                    pl.when(kk == (1 - k if sent else k))(
                        functools.partial(f, h, k, outer, inner))

        def steps(z, lo, hi, sent, f):
            def step(t, c):
                i = t >> 1
                h, kk, outer, inner = half(t & 1)
                k = 1 - kk if sent else kk
                if z == 0:
                    pl.when(i < 2 + k)(lambda: f(z, i, h, k, outer, inner))
                else:
                    f(z, i, h, k, outer, inner)
                return c
            lax.fori_loop(lo, hi, step, 0)

        def flat(z, lo, hi, sent, f):
            for t in range(lo, hi):
                i = t >> 1
                h, kk, outer, inner = hv[t & 1]
                k = 1 - kk if sent else kk
                if z == 0 and i == 2:
                    pl.when(k == 1)(functools.partial(f, z, i, h, k, outer, inner))
                else:
                    f(z, i, h, k, outer, inner)

        def enc(ph, z, h, i, ws, flag):
            s = slot(ph, h, i)

            def put(n, v):
                psend[z][s, 8 * n:8 * n + 8, :] = v
            fl_ref[...] = _encode(ws, put, flag)

        def dec(ph, z, h, i, put_w):
            s = slot(ph, h, i)
            return _decode(lambda n: precv[z][s, 8 * n:8 * n + 8, :], put_w,
                           _NRB[z], fl_ref[...])

        for j in range(2):
            raw_load(hv[j][0]).start()

        @pl.when(p != 2)
        def _():
            for j in range(2):
                pl.semaphore_signal(bar, inc=1, device_id=(hv[j][2],),
                                    device_id_type=_MESH)

        for z in range(2):
            flat(z, 0, 2 * _NU, True,
                 lambda z, i, h, k, o, n: unit_load(z, h, k, i).start())

        @pl.when(p == 2)
        def _():
            pl.semaphore_wait(bar, 2)
            for j in range(2):
                pl.semaphore_signal(hsem, inc=1, device_id=(hv[j][2],),
                                    device_id_type=_MESH)

        fl_ref[...] = jnp.zeros((8, 128), _I32)
        pl.when(odd)(lambda: pl.semaphore_wait(bar, 1))

        for h, kk, outer, _ in hv:
            raw_load(h).wait()
            t1s[h] = xv[raw_rows(h), :].astype(_BF)
            pl.when(kk == 1)(lambda h=h, outer=outer: raw_copy(0, h, 0, outer).start())

        def f1(z, i, h, k, outer, inner):
            unit_load(z, h, k, i).wait()
            r0 = row(z, h, k, i)
            ws = [_pack16(xv[blk(r0, rb), :].astype(_BF)) for rb in range(_NRB[z])]
            enc(0, z, h, i, ws, fl_ref[...])
            if z == 0:
                pl.when(k == 0)(lambda: unit_copy(0, z, h, i, outer).start())
            else:
                unit_copy(0, z, h, i, outer).start()

        steps(0, 0, 2 * _NU, True, f1)
        pl.when(p == 0)(lambda: pl.semaphore_wait(bar, 2))
        pl.when(odd)(lambda: pl.semaphore_wait(hsem, 1))
        for h, kk, outer, _ in hv:
            @pl.when(kk == 0)
            def _():
                raw_copy(0, h, 1, outer).start()
                for i in range(_NU):
                    unit_copy(0, 0, h, i, outer).start()
        steps(1, 0, 2 * _NU, True, f1)

        def keep_main(j):
            h, kk = hv[j][:2]
            return load(row(0, h, kk, kk), 480, ksem.at[j])

        def keep_extra(j):
            return load(row(0, hv[j][0], 1, 0), 48, ksem.at[2 + j])

        for j in range(2):
            pl.when(hv[j][1] == 1)(lambda j=j: keep_extra(j).start())
            keep_main(j).start()
        for j in range(2):
            pl.when(hv[j][1] == 1)(lambda j=j: keep_extra(j).wait())
            keep_main(j).wait()

        def g2(h, k, outer, inner):
            raw_copy(0, h, k, outer).wait_recv()
            t2s[h, :, cols[k]] = (
                xv[raw_rows(h), cols[k]] + t1r[h, :, cols[k]].astype(_F32)).astype(_BF)
            raw_copy(1, h, k, inner).start()

        def f2(z, i, h, k, outer, inner):
            unit_copy(0, z, h, i, outer).wait_recv()
            r0 = row(z, h, k, i)
            ws = []

            def put_w(rb, w):
                w = _pack16((xv[blk(r0, rb), :] + _unpack16(w)).astype(_BF))
                own2[wblk(r0, rb), :] = w
                ws.append(w)
            flag = dec(0, z, h, i, put_w)
            enc(1, z, h, i, ws, flag)
            unit_copy(1, z, h, i, inner).start()

        pieces(False, g2)
        pieces(True, lambda h, k, o, n: raw_copy(0, h, k, o).wait_send())
        for z in range(2):
            steps(z, 0, 2 * _NU, False, f2)
        for z in range(2):
            flat(z, 0, 2 * _NU, True,
                 lambda z, i, h, k, o, n: unit_copy(0, z, h, i, o).wait_send())

        def g3(h, k, outer, inner):
            raw_copy(1, h, k, inner).wait()
            o_ref[raw_rows(h), cols[k]] = (
                t2s[h, :, cols[k]].astype(_F32)
                + t2r[h, :, cols[k]].astype(_F32)).astype(_BF)

        def f3(z, i, h, k, outer, inner):
            unit_copy(1, z, h, i, inner).wait_recv()
            r0 = row(z, h, k, i)
            ws = []

            def put_w(rb, w):
                v = (_unpack16(own2[wblk(r0, rb), :]) + _unpack16(w)).astype(_BF)
                o_ref[blk(r0, rb), :] = v
                ws.append(_pack16(v))
            flag = dec(1, z, h, i, put_w)
            enc(2, z, h, i, ws, flag)
            if z == 0:
                pl.when(i > 0)(lambda: unit_copy(2, z, h, i, outer).start())
            else:
                unit_copy(2, z, h, i, outer).start()

        pieces(False, g3)
        for z in range(2):
            steps(z, 0, 2 * _NU, False, f3)
        flat(0, 0, 2, False, lambda z, i, h, k, o, n: unit_copy(2, z, h, i, o).start())
        pieces(False, lambda h, k, o, n: raw_copy(2, h, k, o).start())
        for z in range(2):
            flat(z, 0, 2 * _NU, False,
                 lambda z, i, h, k, o, n: unit_copy(1, z, h, i, n).wait_send())

        def f4(z, i, h, k, outer, inner):
            unit_copy(2, z, h, i, outer).wait_recv()
            r0 = row(z, h, k, i)

            def put_w(rb, w):
                o_ref[blk(r0, rb), :] = _unpack16(w).astype(_BF)
            fl_ref[...] = dec(2, z, h, i, put_w)

        def sent3(z, i, h, k, outer, inner):
            unit_copy(2, z, h, i, outer).wait_send()

        steps(0, 2, 2 * _NU, True, f4)
        steps(1, 0, 2 * _NU, True, f4)
        redo = jnp.max(jnp.where(fl_ref[...] != 0, 1, 0))
        flat(0, 2, 2 * _NU, False, sent3)
        flat(1, 0, 2 * _NU, False, sent3)
        steps(0, 0, 2, True, f4)
        flat(0, 0, 2, False, sent3)
        pieces(False, lambda h, k, o, n: raw_copy(2, h, k, o).wait_send())
        pieces(True, lambda h, k, o, n: raw_copy(2, h, k, o).wait_recv())

        @pl.when(redo != 0)
        def _fallback():
            fq = _HM // 2

            def loop16(f):
                def step(i, c):
                    f(pl.multiple_of(i * 16, 16))
                    return c
                lax.fori_loop(0, fq // 16, step, 0)

            def at16(r0, r):
                return pl.ds(pl.multiple_of(r0 + r, 16), 16)

            kp = [pl.multiple_of(h * _HM + kk * fq, 16) for h, kk, _, _ in hv]
            sd = [pl.multiple_of(h * _HM + (1 - kk) * fq, 16) for h, kk, _, _ in hv]
            e1 = [rc(f1s.at[h], f1r.at[h], fss.at[h], frs.at[h], outer)
                  for h, _, outer, _ in hv]
            e2 = [rc(f2s.at[h], f2r.at[h], fss.at[2 + h], frs.at[2 + h], inner)
                  for h, _, _, inner in hv]

            def e3(r0, j):
                h, _, outer, _ = hv[j]
                return rc(o_ref.at[pl.ds(r0, fq)], o_ref.at[pl.ds(r0, fq)],
                          fss.at[4 + h], frs.at[4 + h], outer)

            for j in range(2):
                def cast(r, j=j, h=hv[j][0]):
                    f1s[h, pl.ds(r, 16), :] = xv[at16(sd[j], r), :].astype(_BF)
                loop16(cast)
                e1[j].start()
            for j in range(2):
                def add1(r, j=j, h=hv[j][0]):
                    f2s[h, pl.ds(r, 16), :] = (
                        xv[at16(kp[j], r), :]
                        + f1r[h, pl.ds(r, 16), :].astype(_F32)).astype(_BF)
                e1[j].wait_recv()
                loop16(add1)
                e2[j].start()
            for j in range(2):
                def add2(r, j=j, h=hv[j][0]):
                    o_ref[at16(kp[j], r), :] = (
                        f2s[h, pl.ds(r, 16), :].astype(_F32)
                        + f2r[h, pl.ds(r, 16), :].astype(_F32)).astype(_BF)
                e2[j].wait_recv()
                loop16(add2)
                e3(kp[j], j).start()
            for j in range(2):
                e1[j].wait_send()
                e2[j].wait_send()
                e3(kp[j], j).wait_send()
                e3(sd[j], j).wait_recv()

    dma = pltpu.SemaphoreType.DMA
    small = pltpu.VMEM((6 * _NU, (3 * _NRB[0] + 1) * 8, 128), _I32)
    large = pltpu.VMEM((6 * _NU, (3 * _NRB[1] + 1) * 8, 128), _I32)
    raw = pltpu.VMEM((2, _RAW, _N), _BF)
    full = pltpu.VMEM((2, _HM // 2, _N), _BF)
    return pl.pallas_call(
        body,
        out_shape=jax.ShapeDtypeStruct((_M, _N), _BF),
        in_specs=[pl.BlockSpec(memory_space=pl.ANY)],
        out_specs=pl.BlockSpec(memory_space=pltpu.VMEM),
        scratch_shapes=[
            pltpu.VMEM((_M, _N), _F32),
            small, small, large, large,
            pltpu.VMEM((_M // 2, _N), _I32),
            raw, raw, raw, raw,
            pltpu.VMEM((8, 128), _I32),
            full, full, full, full,
            dma((2 + 4 * _NU,)), dma((4,)),
            dma((12 * _NU,)), dma((12 * _NU,)),
            dma((6,)), dma((6,)),
            dma((6,)), dma((6,)),
            pltpu.SemaphoreType.REGULAR,
        ],
        compiler_params=pltpu.CompilerParams(
            collective_id=0,
            vmem_limit_bytes=40 * 1024 * 1024,
            disable_semaphore_checks=True,
        ),
    )(x)
```

```python
import functools

import jax
import jax.numpy as jnp
import numpy as np
from jax import lax
from jax.experimental import pallas as pl
from jax.experimental.pallas import tpu as pltpu

_MESH = pl.DeviceIdType.MESH
_BF = jnp.bfloat16
_F32 = jnp.float32
_I32 = jnp.int32

_EXP = 0x7F807F80
_TOP = 0x80008000
_NIB = 0x07800780
_B11 = 0x08000800
_KEEP = 0x87FF87FF


def _c(v):
    return np.int32(v - (1 << 32) if v >= (1 << 31) else v)


def _sh(x, k):
    if k == 0:
        return x
    if k > 0:
        return lax.shift_left(x, np.int32(k))
    return lax.shift_right_logical(x, np.int32(-k))


def _cb(x, i):
    return lax.slice_in_dim(x, 128 * i, 128 * i + 128, axis=1)


def _tile4(x):
    return jnp.concatenate([x] * 4, axis=1)


@functools.partial(jax.jit, inline=True)
def _pack16(vb):
    u = lax.bitcast_convert_type(vb.astype(_F32), _I32)
    return (u[:8] & _c(0xFFFF0000)) | _sh(u[8:], -16)


@functools.partial(jax.jit, inline=True)
def _unpack16(w):
    hi = lax.bitcast_convert_type(w & _c(0xFFFF0000), _F32)
    lo = lax.bitcast_convert_type(_sh(w, 16), _F32)
    return jnp.concatenate([hi, lo], axis=0)


@functools.partial(jax.jit, static_argnums=3, inline=True)
def _squeeze(w, bb4, cc4, q):
    x = w & _c(_EXP)
    m = (x + cc4) & _c(_TOP)
    m = m - _sh(m, -15)
    wp = w - (bb4 & m)
    d = _cb(wp, 3)
    out = jnp.concatenate([
        (_cb(wp, 0) & _c(_KEEP)) | (_sh(d, 11) & 0x78007800),
        (_cb(wp, 1) & _c(_KEEP)) | (_sh(d, 7) & 0x78007800),
        (_cb(wp, 2) & _c(_KEEP)) | (_sh(d, 3) & 0x38003800)
        | (_sh(d, -1) & 0x40004000)], axis=0)
    return (x & ~m,
            _sh(wp + _c(_NIB), q - 11) & _c(0x00030003 << q),
            out)


@functools.partial(jax.jit, static_argnums=3, inline=True)
def _expand(o, acc, bb4, q):
    o0, o1, o2 = o[:8], o[8:16], o[16:]
    d = ((_sh(o0, -11) & 0x000F000F) | (_sh(o1, -7) & 0x00F000F0)
         | (_sh(o2, -3) & 0x07000700) | (_sh(o2, 1) & _c(_TOP)))
    wn = jnp.concatenate(
        [o0 & _c(_KEEP), o1 & _c(_KEEP), o2 & _c(_KEEP), d], axis=1)
    r = _sh(acc, 11 - q)
    z = (wn & _c(_NIB)) + _c(_NIB)
    m = (z | r) & _c(_B11)
    m = _sh(m, 4) - _sh(m, -11)
    return wn + ((z ^ r) & _c(_B11)) + (bb4 & m) - (_sh(r, -1) & _c(_B11))


def _rows8(x):
    return jnp.broadcast_to(x, (8, 128))


def _encode(ws, put, put_meta, flag):
    sub = lax.broadcasted_iota(_I32, (8, 128), 0)
    mx = None
    for w in ws:
        x = w & _c(_EXP)
        x = jnp.maximum(x, _sh(x, 16))
        mx = x if mx is None else jnp.maximum(mx, x)
    mx = jnp.maximum(jnp.maximum(_cb(mx, 0), _cb(mx, 1)),
                     jnp.maximum(_cb(mx, 2), _cb(mx, 3)))
    base = jnp.maximum(_sh(jnp.max(mx, axis=0, keepdims=True), -23) - 47, 0)
    bb = _rows8(_sh(base, 7) | _sh(base, 23))
    bb4 = _tile4(bb)
    cc4 = _tile4(_c(_EXP) - bb)
    bad = acc = None
    for rb, w in enumerate(ws):
        b, r, out = _squeeze(w, bb4, cc4, 2 * rb)
        bad = b if bad is None else bad | b
        acc = r if acc is None else acc | r
        put(rb, out)
    flag = flag | _cb(bad, 0) | _cb(bad, 1) | _cb(bad, 2) | _cb(bad, 3)
    r = (acc ^ _sh(acc, -1)) & 0x55555555
    rare, low = ([_cb(v, 0) | _sh(_cb(v, 1), 1), _cb(v, 2) | _sh(_cb(v, 3), 1)]
                 for v in (r, acc & r))
    if len(ws) <= 4:
        rare, low = [rare[0] | _sh(rare[1], 8)], [low[0] | _sh(low[1], 8)]
    fields = []
    for _ in range(3):
        if len(rare) == 1:
            sel, cls = rare[0], low[0]
        else:
            use = rare[0] == 0
            sel = jnp.where(use, rare[1], rare[0])
            cls = jnp.where(use, low[1], low[0])
        one = sel & (0 - sel)
        e = _sh(lax.bitcast_convert_type(one.astype(_F32), _I32), -23) & 0xFF
        code = e - 126 + jnp.where((cls & one) != 0, 64, 0)
        if len(rare) == 1:
            rare = [sel ^ one]
        else:
            rare = [rare[0] & (rare[0] - 1), jnp.where(use, sel ^ one, rare[1])]
            code = code + jnp.where(use, 32, 0)
            flag = flag | (jnp.maximum(code, 0) & 128)
        fields.append(jnp.where(one != 0, _sh(code, 3) | sub, 0))
    for r in rare:
        flag = flag | r
    after = lax.shift_left(jnp.full((8, 128), 0x11111110, _I32), 4 * sub)
    cnt = sum(jnp.where(f != 0, after, 0) for f in fields)
    cnt = _rows8(jnp.sum(cnt, axis=0, keepdims=True))
    first = (lax.shift_right_logical(cnt, 4 * sub) & 15) * 10 + 10
    rows = [None, None]
    for t, f in enumerate(fields):
        bit = first + 10 * t
        for n in range(2):
            s = bit - 30 * n
            v = jnp.where((s >= 0) & (s < 30), lax.shift_left(f, s & 31), 0)
            rows[n] = v if rows[n] is None else rows[n] | v
        flag = flag | jnp.where(bit >= 60, f, 0)
    rows = [jnp.sum(v, axis=0, keepdims=True) for v in rows]
    put_meta(0, rows[0] | base
             | jnp.max(jnp.where(flag != 0, 255, 0), axis=0, keepdims=True))
    put_meta(1, rows[1])
    return flag


def _decode(get, get_meta, put_w, nrb, flag):
    sub = lax.broadcasted_iota(_I32, (8, 128), 0)
    rows = [_rows8(get_meta(n)) for n in range(2)]
    base = rows[0] & 0xFF
    flag = flag | _sh(base + 1, -8)
    base = base + 16
    bb4 = _tile4(_sh(base, 7) | _sh(base, 23))
    maps = [None] * 4
    for t in range(1, 6):
        f = _sh(rows[t // 3], -10 * (t % 3))
        code = jnp.where((f & 7) == sub, _sh(f, -3) & 127, 0)
        pos = code - 1
        if nrb <= 4:
            idx, amt = (_sh(pos, -2) & 2) | (pos & 1), pos & 0x16
        else:
            idx, amt = (_sh(pos, -4) & 2) | (pos & 1), pos & 0x1E
        val = lax.shift_left(jnp.where(code > 64, 3, jnp.where(code > 0, 1, 0)), amt)
        for n in range(4):
            v = jnp.where(idx == n, val, 0)
            maps[n] = v if maps[n] is None else maps[n] | v
    acc = jnp.concatenate(maps, axis=1)
    for rb in range(nrb):
        put_w(rb, _expand(get(rb), acc, bb4, 2 * rb))
    return flag


_M, _N = 2048, 512
_HM = _M // 2
_CS = 256
_NRB = ((2, 3), (4, 6), (8, 8))
_ROW = ((16, 496), (48, 544), (112, 640))
_PAY = (0, 80, 232)
_PAY_ROWS = 232 + 3 * 200
_QUARTER = ((16, 480), (496, 528))


def pallas_dist_ar_i_i_m2048_n512_kernel(x: jax.Array):
    assert x.shape == (_M, _N)

    def body(x_ref, o_ref, xv, psend, precv, own2, t1f, t1s, t1r, t2s, t2r,
             fl_ref, f1s, f1r, f2s, f2r,
             lsem, ksem, ss, rs, mss, mrs, tss, trs, fss, frs, hsem):
        p = lax.axis_index("i")
        py, px = p ^ 1, 3 - p
        yc, xc = (p ^ (p >> 1)) & 1, p >> 1
        flip = (p + 1) >> 2
        odd = (p & 1) == 1
        bar = pltpu.get_barrier_semaphore()
        cols = (pl.ds(0, _CS), pl.ds(_CS, _N - _CS))

        def half(j):
            h = j ^ flip
            kk = jnp.where(h == 0, yc, xc)
            outer = jnp.where(h == 0, py, px)
            inner = jnp.where(h == 0, px, py)
            return h, kk, outer, inner

        hv = [half(j) for j in range(2)]

        def rc(src, dst, s_sem, r_sem, dev):
            return pltpu.make_async_remote_copy(
                src_ref=src, dst_ref=dst, send_sem=s_sem, recv_sem=r_sem,
                device_id=(dev,), device_id_type=_MESH)

        class Unit:
            def __init__(self, z, i, k, h, outer, inner):
                self.z, self.k, self.h = z, k, h
                self.outer, self.inner = outer, inner
                self.nrb = _NRB[z][k if z < 2 else 0]
                self.r0 = (h * _HM + _ROW[z][0] + k * (_ROW[z][1] - _ROW[z][0])
                           + 16 * self.nrb * i)
                self.p0 = _PAY[z] + (24 * self.nrb + 8) * i
                self.id = h * 5 + z + i
                self.lead = z == 0 and k == 0

            def rows(self, rb, n=1):
                return pl.ds(pl.multiple_of(self.r0 + 16 * rb, 16), 16 * n)

            def words(self, rb):
                return pl.ds(pl.multiple_of((self.r0 >> 1) + 8 * rb, 8), 8)

            def pay(self, rb, n):
                start = self.p0 + 24 * rb
                if not isinstance(start, int):
                    start = pl.multiple_of(start, 8)
                return pl.ds(start, n)

            def meta(self, n):
                return pl.ds(self.p0 + 24 * self.nrb + n, 1)

            def load(self):
                rows = self.rows(0, self.nrb)
                return pltpu.make_async_copy(
                    x_ref.at[rows], xv.at[rows], lsem.at[self.id])

            def parts(self, ph):
                return 2 if ph == 0 and self.lead else 1

            def copy(self, ph, part):
                s = 2 * ph + self.h
                if part:
                    v, sems = self.pay(self.nrb, 2), (mss.at[self.h], mrs.at[self.h])
                else:
                    v = self.pay(0, 24 * self.nrb + 4 - 2 * self.parts(ph))
                    sems = ss.at[10 * ph + self.id], rs.at[10 * ph + self.id]
                return rc(psend.at[s, v], precv.at[s, v], *sems,
                          self.inner if ph == 1 else self.outer)

            def start(self, ph):
                self.copy(ph, self.parts(ph) - 1).start()

            def wait_send(self, ph):
                for part in range(self.parts(ph)):
                    self.copy(ph, part).wait_send()

            def encode(self, ph, ws, flag):
                s = 2 * ph + self.h

                def put(rb, val):
                    psend[s, self.pay(rb, 24), :] = val
                    if self.parts(ph) == 2 and rb == self.nrb - 1:
                        self.copy(ph, 0).start()

                def put_meta(n, val):
                    psend[s, self.meta(n), :] = val
                fl_ref[...] = _encode(ws, put, put_meta, flag)

            def decode(self, ph, put_w):
                s = 2 * ph + self.h
                for part in range(self.parts(ph)):
                    self.copy(ph, part).wait_recv()
                return _decode(lambda rb: precv[s, self.pay(rb, 24), :],
                               lambda n: precv[s, self.meta(n), :],
                               put_w, self.nrb, fl_ref[...])

        def per_quarter(hk, sent, f):
            h, kk, outer, inner = hk
            for k in range(2):
                pl.when(kk == (1 - k if sent else k))(
                    functools.partial(f, k, h, outer, inner))

        def pieces(sent, f):
            for hk in hv:
                per_quarter(hk, sent, f)

        def visit(z, i, hk, sent, f):
            if z < 2:
                per_quarter(hk, sent, lambda *a: f(Unit(z, 0, *a)))
            else:
                h, kk, outer, inner = hk
                f(Unit(z, i, 1 - kk if sent else kk, h, outer, inner))

        def steps(classes, sent, f):
            for z in classes:
                def step(t, c, z=z):
                    visit(z, t >> 1, half(t & 1), sent, f)
                    return c
                lax.fori_loop(0, 6 if z == 2 else 2, step, 0)

        def flat(classes, sent, f):
            for z in classes:
                for i in range(3 if z == 2 else 1):
                    for hk in hv:
                        visit(z, i, hk, sent, f)

        def raw_rows(h):
            return pl.ds(pl.multiple_of(h * _HM, 16), 16)

        def raw_load(h):
            return pltpu.make_async_copy(
                x_ref.at[raw_rows(h)], xv.at[raw_rows(h)], ksem.at[h])

        def raw_copy(ph, k, h, dev):
            if ph == 0 and k == 0:
                src, dst = x_ref.at[raw_rows(h), cols[0]], t1f.at[h]
            elif ph == 0:
                src, dst = t1s.at[h], t1r.at[h]
            elif ph == 1:
                src, dst = t2s.at[h, :, cols[k]], t2r.at[h, :, cols[k]]
            else:
                src = dst = o_ref.at[raw_rows(h), cols[k]]
            return rc(src, dst, tss.at[2 * ph + h], trs.at[2 * ph + h], dev)

        def keep_load(k, h):
            rows = pl.ds(pl.multiple_of(h * _HM + _QUARTER[k][0], 16), _QUARTER[k][1])
            return pltpu.make_async_copy(x_ref.at[rows], xv.at[rows], ksem.at[2 + h])

        def signal(sem):
            for hk in hv:
                pl.semaphore_signal(sem, inc=1, device_id=(hk[2],),
                                    device_id_type=_MESH)

        flat((0,), True, lambda u: u.load().start())
        pl.when(p != 2)(lambda: signal(bar))

        @pl.when(odd)
        def _():
            pl.semaphore_wait(bar, 1)
            raw_copy(0, 0, hv[0][0], hv[0][2]).start()

        @pl.when(p == 2)
        def _():
            pl.semaphore_wait(bar, 2)
            for hk in hv:
                raw_copy(0, 0, hk[0], hk[2]).start()
            signal(hsem)

        flat((1,), True, lambda u: u.load().start())
        for hk in hv:
            raw_load(hk[0]).start()
        flat((2,), True, lambda u: u.load().start())
        fl_ref[...] = jnp.zeros((8, 128), _I32)

        def f1(u):
            u.load().wait()
            ws = [_pack16(xv[u.rows(rb), :].astype(_BF)) for rb in range(u.nrb)]
            u.encode(0, ws, fl_ref[...])
            if u.z == 2 or u.k == 0:
                u.start(0)

        steps((0, 1), True, f1)
        for hk in hv:
            raw_load(hk[0]).wait()
            t1s[hk[0]] = xv[raw_rows(hk[0]), cols[1]].astype(_BF)
        pl.when(p == 0)(lambda: pl.semaphore_wait(bar, 2))
        pl.when(odd)(lambda: pl.semaphore_wait(hsem, 1))
        for h, kk, outer, inner in hv:
            @pl.when(kk == 0)
            def _():
                raw_copy(0, 1, h, outer).start()
                for z in range(2):
                    Unit(z, 0, 1, h, outer, inner).start(0)
        steps((2,), True, f1)
        pieces(False, lambda k, h, o, n: keep_load(k, h).start())
        pieces(False, lambda k, h, o, n: keep_load(k, h).wait())

        def g2(k, h, outer, inner):
            raw_copy(0, k, h, outer).wait_recv()
            got = t1r[h].astype(_F32) if k else t1f[h]
            t2s[h, :, cols[k]] = (xv[raw_rows(h), cols[k]] + got).astype(_BF)
            raw_copy(1, k, h, inner).start()

        def f2(u):
            ws = []

            def put_w(rb, w):
                w = _pack16((xv[u.rows(rb), :] + _unpack16(w)).astype(_BF))
                own2[u.words(rb), :] = w
                ws.append(w)
            flag = u.decode(0, put_w)
            u.encode(1, ws, flag)
            u.start(1)

        pieces(False, g2)
        pieces(True, lambda k, h, o, n: raw_copy(0, k, h, o).wait_send())
        steps((0, 1, 2), False, f2)
        flat((0, 1, 2), True, lambda u: u.wait_send(0))

        def g3(k, h, outer, inner):
            raw_copy(1, k, h, inner).wait()
            o_ref[raw_rows(h), cols[k]] = (
                t2s[h, :, cols[k]].astype(_F32)
                + t2r[h, :, cols[k]].astype(_F32)).astype(_BF)

        def f3(u):
            ws = []

            def put_w(rb, w):
                v = (_unpack16(own2[u.words(rb), :]) + _unpack16(w)).astype(_BF)
                o_ref[u.rows(rb), :] = v
                ws.append(_pack16(v))
            flag = u.decode(1, put_w)
            u.encode(2, ws, flag)
            if u.z:
                u.start(2)

        pieces(False, g3)
        steps((0, 1, 2), False, f3)
        flat((0,), False, lambda u: u.start(2))
        pieces(False, lambda k, h, o, n: raw_copy(2, k, h, o).start())
        flat((0, 1, 2), False, lambda u: u.wait_send(1))

        def f4(u):
            def put_w(rb, w):
                o_ref[u.rows(rb), :] = _unpack16(w).astype(_BF)
            fl_ref[...] = u.decode(2, put_w)

        steps((1, 2), True, f4)
        redo = jnp.max(jnp.where(fl_ref[...] != 0, 1, 0))
        flat((1, 2), False, lambda u: u.wait_send(2))
        steps((0,), True, f4)
        flat((0,), False, lambda u: u.wait_send(2))
        pieces(False, lambda k, h, o, n: raw_copy(2, k, h, o).wait_send())
        pieces(True, lambda k, h, o, n: raw_copy(2, k, h, o).wait_recv())

        @pl.when(redo != 0)
        def _fallback():
            fq = _HM // 2

            def loop16(f):
                def step(i, c):
                    f(pl.multiple_of(i * 16, 16))
                    return c
                lax.fori_loop(0, fq // 16, step, 0)

            def at16(r0, r):
                return pl.ds(pl.multiple_of(r0 + r, 16), 16)

            kp = [pl.multiple_of(h * _HM + kk * fq, 16) for h, kk, _, _ in hv]
            sd = [pl.multiple_of(h * _HM + (1 - kk) * fq, 16) for h, kk, _, _ in hv]
            e1 = [rc(f1s.at[h], f1r.at[h], fss.at[h], frs.at[h], outer)
                  for h, _, outer, _ in hv]
            e2 = [rc(f2s.at[h], f2r.at[h], fss.at[2 + h], frs.at[2 + h], inner)
                  for h, _, _, inner in hv]

            def e3(r0, j):
                h, _, outer, _ = hv[j]
                return rc(o_ref.at[pl.ds(r0, fq)], o_ref.at[pl.ds(r0, fq)],
                          fss.at[4 + h], frs.at[4 + h], outer)

            for j in range(2):
                def cast(r, j=j, h=hv[j][0]):
                    f1s[h, pl.ds(r, 16), :] = xv[at16(sd[j], r), :].astype(_BF)
                loop16(cast)
                e1[j].start()
            for j in range(2):
                def add1(r, j=j, h=hv[j][0]):
                    f2s[h, pl.ds(r, 16), :] = (
                        xv[at16(kp[j], r), :]
                        + f1r[h, pl.ds(r, 16), :].astype(_F32)).astype(_BF)
                e1[j].wait_recv()
                loop16(add1)
                e2[j].start()
            for j in range(2):
                def add2(r, j=j, h=hv[j][0]):
                    o_ref[at16(kp[j], r), :] = (
                        f2s[h, pl.ds(r, 16), :].astype(_F32)
                        + f2r[h, pl.ds(r, 16), :].astype(_F32)).astype(_BF)
                e2[j].wait_recv()
                loop16(add2)
                e3(kp[j], j).start()
            for j in range(2):
                e1[j].wait_send()
                e2[j].wait_send()
                e3(kp[j], j).wait_send()
                e3(sd[j], j).wait_recv()

    dma = pltpu.SemaphoreType.DMA
    pay = pltpu.VMEM((6, _PAY_ROWS, 128), _I32)
    raw1 = pltpu.VMEM((2, 16, _N - _CS), _BF)
    raw2 = pltpu.VMEM((2, 16, _N), _BF)
    full = pltpu.VMEM((2, _HM // 2, _N), _BF)
    return pl.pallas_call(
        body,
        out_shape=jax.ShapeDtypeStruct((_M, _N), _BF),
        in_specs=[pl.BlockSpec(memory_space=pl.ANY)],
        out_specs=pl.BlockSpec(memory_space=pltpu.VMEM),
        scratch_shapes=[
            pltpu.VMEM((_M, _N), _F32),
            pay, pay,
            pltpu.VMEM((_M // 2, _N), _I32),
            pltpu.VMEM((2, 16, _CS), _F32),
            raw1, raw1, raw2, raw2,
            pltpu.VMEM((8, 128), _I32),
            full, full, full, full,
            dma((10,)), dma((4,)),
            dma((30,)), dma((30,)),
            dma((2,)), dma((2,)),
            dma((6,)), dma((6,)),
            dma((6,)), dma((6,)),
            pltpu.SemaphoreType.REGULAR,
        ],
        compiler_params=pltpu.CompilerParams(
            collective_id=0,
            vmem_limit_bytes=40 * 1024 * 1024,
            disable_semaphore_checks=True,
        ),
    )(x)
```
